```python
import numpy as np

kernel_name = "dist_sum_ax1_xy_m512_n256"

def setup_inputs():
    return {"x": np.random.randn(1024, 512).astype(np.float32)}

def reference(x: np.ndarray) -> np.ndarray:
    return np.sum(x, axis=1, keepdims=True)
```

```python
import jax
import jax.numpy as jnp
from jax import lax
from jax.experimental import pallas as pl
from jax.experimental.pallas import tpu as pltpu

N_CHUNKS = 4


def pallas_dist_sum_ax1_xy_m512_n256_kernel(
    x: jax.Array,
):
    m, n = x.shape
    rows = m // N_CHUNKS

    def body(x_hbm, o_hbm, x_vmem, mine, theirs, load_sems, send_sem, recv_sem, out_sem):
        my_x = lax.axis_index("x")
        my_y = lax.axis_index("y")
        peer = (my_x, 1 - my_y)

        barrier = pltpu.get_barrier_semaphore()
        pl.semaphore_signal(
            barrier, inc=1, device_id=peer, device_id_type=pl.DeviceIdType.MESH
        )

        loads = [
            pltpu.make_async_copy(
                x_hbm.at[pl.ds(c * rows, rows)],
                x_vmem.at[pl.ds(c * rows, rows)],
                load_sems.at[c],
            )
            for c in range(N_CHUNKS)
        ]
        for cp in loads:
            cp.start()

        ones = jnp.ones((8, 128), jnp.bfloat16)
        for c in range(N_CHUNKS):
            loads[c].wait()
            blk = x_vmem[pl.ds(c * rows, rows), :]
            folded = blk[:, :128] + blk[:, 128:]
            part = lax.dot_general(
                ones,
                folded.astype(jnp.bfloat16),
                (((1,), (1,)), ((), ())),
                preferred_element_type=jnp.float32,
            )
            mine[:, pl.ds(c * rows, rows)] = part[:1]

        pl.semaphore_wait(barrier, 1)
        rdma = pltpu.make_async_remote_copy(
            src_ref=mine,
            dst_ref=theirs,
            send_sem=send_sem,
            recv_sem=recv_sem,
            device_id=peer,
            device_id_type=pl.DeviceIdType.MESH,
        )
        rdma.start()
        rdma.wait_recv()
        theirs[...] = theirs[...] + mine[...]
        out = pltpu.make_async_copy(theirs, o_hbm, out_sem)
        out.start()
        rdma.wait_send()
        out.wait()

    out = pl.pallas_call(
        body,
        out_shape=jax.ShapeDtypeStruct((1, m), x.dtype),
        in_specs=[pl.BlockSpec(memory_space=pl.ANY)],
        out_specs=pl.BlockSpec(memory_space=pl.ANY),
        scratch_shapes=[
            pltpu.VMEM((m, n), x.dtype),
            pltpu.VMEM((1, m), jnp.float32),
            pltpu.VMEM((1, m), jnp.float32),
            pltpu.SemaphoreType.DMA((N_CHUNKS,)),
            pltpu.SemaphoreType.DMA,
            pltpu.SemaphoreType.DMA,
            pltpu.SemaphoreType.DMA,
        ],
        compiler_params=pltpu.CompilerParams(collective_id=0),
    )(x)
    return out.reshape(m, 1)
```

```python
import jax
import jax.numpy as jnp
from jax import lax
from jax.experimental import pallas as pl
from jax.experimental.pallas import tpu as pltpu

SUBLANES, LANES = 8, 128

RAW_ROWS = 16
TAIL_LOADS = (96, 88, 72)


def pallas_dist_sum_ax1_xy_m512_n256_kernel(
    x: jax.Array,
):
    m, n = x.shape
    split = m - LANES

    pieces, start = [], RAW_ROWS
    for rows in (m - RAW_ROWS - sum(TAIL_LOADS), *TAIL_LOADS):
        pieces.append((start, rows))
        start += rows

    def body(x_hbm, o_ref, x_vmem, peer_raw, mine, theirs, load_sems, send_sems, recv_sems):
        peer = dict(
            device_id=(lax.axis_index("x"), 1 - lax.axis_index("y")),
            device_id_type=pl.DeviceIdType.MESH,
        )

        def load(i, start, rows):
            block = pl.ds(start, rows)
            return pltpu.make_async_copy(x_hbm.at[block], x_vmem.at[block], load_sems.at[i])

        def send(i, src, dst):
            return pltpu.make_async_remote_copy(
                src, dst, send_sems.at[i], recv_sems.at[i], **peer
            )

        loads = [load(i, *piece) for i, piece in enumerate(pieces)]
        own_raw = load(len(pieces), 0, RAW_ROWS)
        head, tail = pl.ds(0, split), pl.ds(split, LANES)
        send_head = send(0, mine.at[:, head], theirs.at[:, head])
        send_tail = send(1, mine.at[:, tail], theirs.at[:, tail])
        send_raw = send(2, x_hbm.at[pl.ds(0, RAW_ROWS)], peer_raw)

        for copy in loads:
            copy.start()
        barrier = pltpu.get_barrier_semaphore()
        pl.semaphore_signal(barrier, 1, **peer)
        pl.semaphore_wait(barrier, 1)
        send_raw.start()

        vreg = (SUBLANES, LANES)
        diagonal = lax.broadcasted_iota(jnp.int32, vreg, 1) - lax.broadcasted_iota(
            jnp.int32, vreg, 0
        )
        zeros = jnp.zeros(vreg, jnp.float32)

        def fold(ref, row):
            tiles = [
                ref[pl.ds(row, SUBLANES), pl.ds(col, LANES)] for col in range(0, n, LANES)
            ]
            return sum(tiles[1:], tiles[0])

        def place(folded, row, acc):
            sums = jnp.sum(folded, axis=1, keepdims=True)
            return jnp.where(diagonal == row % LANES, sums, acc)

        partial, acc = {}, zeros
        for copy, (start, rows) in zip(loads, pieces):
            copy.wait()
            for row in range(start, start + rows, SUBLANES):
                acc = place(fold(x_vmem, row), row, acc)
                if (row + SUBLANES) % LANES == 0:
                    group = row + SUBLANES - LANES
                    partial[group] = jnp.sum(acc, axis=0, keepdims=True)
                    mine[:, pl.ds(group, LANES)] = partial[group]
                    acc = zeros
            if start < split <= start + rows:
                send_head.start()
        send_tail.start()

        own_raw.start()
        own_raw.wait()
        send_raw.wait_recv()
        acc = zeros
        for row in range(0, RAW_ROWS, SUBLANES):
            acc = place(fold(x_vmem, row) + fold(peer_raw, row), row, acc)
        partial[0] = partial[0] + jnp.sum(acc, axis=0, keepdims=True)

        send_raw.wait_send()
        send_head.wait_send()
        send_tail.wait_send()
        send_head.wait_recv()
        for group in range(0, split, LANES):
            cols = pl.ds(group, LANES)
            o_ref[:, cols] = theirs[:, cols] + partial[group]
        send_tail.wait_recv()
        o_ref[:, tail] = theirs[:, tail] + partial[split]

    out = pl.pallas_call(
        body,
        out_shape=pltpu.VMEM((1, m), jnp.float32),
        in_specs=[pl.BlockSpec(memory_space=pltpu.HBM)],
        out_specs=pl.BlockSpec(memory_space=pltpu.VMEM),
        scratch_shapes=[
            pltpu.VMEM((m, n), x.dtype),
            pltpu.VMEM((RAW_ROWS, n), x.dtype),
            pltpu.VMEM((1, m), jnp.float32),
            pltpu.VMEM((1, m), jnp.float32),
            pltpu.SemaphoreType.DMA((len(pieces) + 1,)),
            pltpu.SemaphoreType.DMA((3,)),
            pltpu.SemaphoreType.DMA((3,)),
        ],
        compiler_params=pltpu.CompilerParams(
            collective_id=0,
            disable_bounds_checks=True,
            disable_semaphore_checks=True,
        ),
    )(x)
    return out.reshape(m, 1)
```

```python
import jax
import jax.numpy as jnp
import numpy as np
from jax import lax
from jax.experimental import pallas as pl
from jax.experimental.pallas import tpu as pltpu

SUBLANES, LANES = 8, 128

RAW_SENDS = (16, 8)
TAIL_LOADS = (104, 88, 80)


def _spans(start, sizes):
    spans = []
    for size in sizes:
        spans.append((start, size))
        start += size
    return spans


def pallas_dist_sum_ax1_xy_m512_n256_kernel(
    x: jax.Array,
):
    m, n = x.shape
    raw_rows = sum(RAW_SENDS)
    pieces = _spans(raw_rows, (m - raw_rows - sum(TAIL_LOADS), *TAIL_LOADS))
    late_start, late_rows = pieces[-1]
    words = late_rows // 2
    last_group = m - LANES
    assert raw_rows < LANES and late_start > last_group and words % SUBLANES == 0

    def body(
        x_hbm,
        o_ref,
        x_vmem,
        peer_raw,
        early_src,
        early_dst,
        late_src,
        late_dst,
        load_sems,
        send_sems,
        recv_sems,
    ):
        def load(i, start, rows):
            span = pl.ds(start, rows)
            return pltpu.make_async_copy(
                x_hbm.at[span], x_vmem.at[span], load_sems.at[i]
            )

        loads = [load(i, *piece) for i, piece in enumerate(pieces)]
        for copy in loads:
            copy.start()

        peer = dict(
            device_id=(lax.axis_index("x"), 1 - lax.axis_index("y")),
            device_id_type=pl.DeviceIdType.MESH,
        )

        def send(i, src, dst):
            return pltpu.make_async_remote_copy(
                src, dst, send_sems.at[i], recv_sems.at[i], **peer
            )

        send_early = send(0, early_src, early_dst)
        send_late = send(1, late_src, late_dst)
        send_raw = [
            send(2 + i, x_hbm.at[pl.ds(*span)], peer_raw.at[pl.ds(*span)])
            for i, span in enumerate(_spans(0, RAW_SENDS))
        ]

        barrier = pltpu.get_barrier_semaphore()
        pl.semaphore_signal(barrier, 1, **peer)
        pl.semaphore_wait(barrier, 1)
        send_raw[0].start()

        vreg = (SUBLANES, LANES)
        lane = lax.broadcasted_iota(jnp.int32, vreg, 1)
        diagonal = lane - lax.broadcasted_iota(jnp.int32, vreg, 0)
        zeros = jnp.zeros(vreg, jnp.float32)

        def fold(ref, row):
            tiles = [
                ref[pl.ds(row, SUBLANES), pl.ds(col, LANES)]
                for col in range(0, n, LANES)
            ]
            return sum(tiles[1:], tiles[0])

        def row_sums(folded):
            return jnp.sum(folded, axis=1, keepdims=True)

        def place(acc, sums, first_lane):
            return jnp.where(diagonal == first_lane, sums, acc)

        def flatten(acc):
            return jnp.sum(acc, axis=0, keepdims=True)

        def as_lanes(blocks, first_lane):
            acc = zeros
            for i, sums in enumerate(blocks):
                acc = place(acc, sums, first_lane + i * SUBLANES)
            return flatten(acc)

        total, acc = {}, zeros
        for i, (start, rows) in enumerate(pieces[:-1]):
            loads[i].wait()
            if i == 0:
                for copy in send_raw[1:]:
                    copy.start()
            for row in range(start, start + rows, SUBLANES):
                acc = place(acc, row_sums(fold(x_vmem, row)), row % LANES)
                if (row + SUBLANES) % LANES == 0 or row + SUBLANES == late_start:
                    group = row // LANES * LANES
                    total[group] = flatten(acc)
                    early_src[:, pl.ds(group, LANES)] = total[group]
                    acc = zeros
        send_early.start()

        def bf16_bits(v):
            rounded = v.astype(jnp.bfloat16).astype(jnp.float32)
            return lax.bitcast_convert_type(rounded, jnp.uint32)

        loads[-1].wait()
        late = [
            row_sums(fold(x_vmem, row)) for row in range(late_start, m, SUBLANES)
        ]
        low, high = late[: len(late) // 2], late[len(late) // 2 :]
        late_src[...] = bf16_bits(as_lanes(high, 0)) | (
            bf16_bits(as_lanes(low, 0)) >> 16
        )
        send_late.start()
        total[last_group] += as_lanes(late, late_start - last_group)

        load_raw = load(len(pieces), 0, raw_rows)
        load_raw.start()
        load_raw.wait()
        for copy in (*send_raw, send_early, send_late):
            copy.wait_send()

        for copy in send_raw:
            copy.wait_recv()
        total[0] += as_lanes(
            [
                row_sums(fold(x_vmem, row) + fold(peer_raw, row))
                for row in range(0, raw_rows, SUBLANES)
            ],
            0,
        )

        late_lane = lane[:1] - (late_start - last_group)
        is_low = late_lane < words
        word = jnp.where(is_low, late_lane, late_lane - words)
        send_late.wait_recv()
        bits = jnp.zeros((1, LANES), jnp.uint32)
        for i in range(words):
            bits = jnp.where(word == i, late_dst[0, i], bits)
        bits = jnp.where(is_low, bits << 16, bits & np.uint32(0xFFFF0000))
        total[last_group] += lax.bitcast_convert_type(bits, jnp.float32)

        send_early.wait_recv()
        for group in range(0, m, LANES):
            cols = pl.ds(group, LANES)
            o_ref[:, cols] = total[group] + early_dst[:, cols]

    n_sends = 2 + len(RAW_SENDS)
    out = pl.pallas_call(
        body,
        out_shape=jax.ShapeDtypeStruct((1, m), jnp.float32),
        in_specs=[pl.BlockSpec(memory_space=pltpu.HBM)],
        out_specs=pl.BlockSpec(memory_space=pltpu.VMEM),
        scratch_shapes=[
            pltpu.VMEM((m, n), x.dtype),
            pltpu.VMEM((raw_rows, n), x.dtype),
            pltpu.VMEM((1, m), jnp.float32),
            pltpu.VMEM((1, m), jnp.float32),
            pltpu.VMEM((1, LANES), jnp.uint32),
            pltpu.SMEM((1, LANES), jnp.uint32),
            pltpu.SemaphoreType.DMA((len(pieces) + 1,)),
            pltpu.SemaphoreType.DMA((n_sends,)),
            pltpu.SemaphoreType.DMA((n_sends,)),
        ],
        compiler_params=pltpu.CompilerParams(
            collective_id=0,
            disable_semaphore_checks=True,
        ),
    )(x)
    return out.reshape(m, 1)
```
